```python
import numpy as np

kernel_name = "dist_sparse_attn_strided_qseq_b1_sq1024_skv1024_hq8_dh128"

def setup_inputs():
    x = np.random.randn(1, 4096, 1024).astype(np.float32)
    Wq = np.random.randn(1024, 4096).astype(np.float32) * 0.02
    K_ext = np.random.randn(1, 1024, 32, 128).astype(np.float32)
    V_ext = np.random.randn(1, 1024, 32, 128).astype(np.float32)
    Wo = np.random.randn(4096, 1024).astype(np.float32) * 0.02
    return {"x": x, "Wq": Wq, "K_ext": K_ext, "V_ext": V_ext, "Wo": Wo}

def reference(x, Wq, K_ext, V_ext, Wo):
    B, Sq, Skv, Hq, Dh = 1, 4096, 1024, 32, 128
    Q = (x @ Wq).reshape(B, Sq, Hq, Dh)
    qb = (np.arange(Sq) // 64)[:, None]
    kb = (np.arange(Skv) // 64)[None, :]
    mask = (qb == kb) | ((kb % 4) == (qb % 4))
    scores = np.einsum('bihd,bjhd->bhij', Q, K_ext).astype(np.float32) * 0.08838834764831843
    scores = np.where(mask[None, None, :, :], scores, -1e9)
    scores_max = scores.max(axis=-1, keepdims=True)
    w = np.exp(scores - scores_max)
    row_keep = mask.any(axis=1)
    w_sum = np.where(row_keep[None, None, :, None], w.sum(axis=-1, keepdims=True), 1.0)
    w = w / w_sum
    w = np.where(row_keep[None, None, :, None], w, 0.0)
    ctx = np.einsum('bhij,bjhd->bihd', w, V_ext).reshape(B, Sq, Hq * Dh)
    return ctx @ Wo
```

```python
import functools
import numpy as np
import jax
import jax.numpy as jnp
from jax import lax
from jax.experimental import pallas as pl
from jax.experimental.pallas import tpu as pltpu

BF = jnp.bfloat16
F32 = jnp.float32
SCALE = 0.08838834764831843 * 1.4426950408889634
NT = (((1,), (1,)), ((), ()))


def _orders():
    kk = [(0, c, 0, g) for c in range(4) for g in range(4)]
    q2 = []
    for t in range(4):
        q2 += [(1, t, 0, g) for g in range(4)]
        q2 += [(1, t, 1, g) for g in range(t)] + [(1, c, 1, t) for c in range(t + 1)]
        q2 += [(0, c, 1, t) for c in range(4)]
    a2 = kk + [it for it in q2 if it[0] == 1]
    a3 = [it for it in q2 if it[0] == 0]
    return kk, q2, a2, a3


def _body(tab, x_hbm, wq_hbm, k_hbm, v_hbm, wo_hbm, out_hbm,
          xf, wqf, wof, kf, vf, xb, wqb, wob, kb, vb, qb, ctx, psend, precv, obuf,
          lsem, ssem, rsem, osem):
    me = lax.axis_index("i")
    pp = me ^ 1
    qq = 3 - me
    kk, q2, a2, a3 = _orders()

    bar = pltpu.get_barrier_semaphore()
    for d in (pp, qq):
        pl.semaphore_signal(bar, inc=1, device_id=(d,), device_id_type=pl.DeviceIdType.MESH)

    def ld_x(c):
        return pltpu.make_async_copy(x_hbm.at[:, c], xf.at[c], lsem.at[c])

    def ld_wq(g):
        return pltpu.make_async_copy(wq_hbm.at[:, pl.ds(256 * g, 256)], wqf.at[g], lsem.at[4 + g])

    def ld_wo(g):
        return pltpu.make_async_copy(wo_hbm.at[:, pl.ds(256 * g, 256)], wof.at[g], lsem.at[8 + g])

    def ld_kv(s, c):
        hb = me if s == 0 else qq
        return (pltpu.make_async_copy(k_hbm.at[:, c, :, hb], kf.at[s, c], lsem.at[12 + 8 * s + c]),
                pltpu.make_async_copy(v_hbm.at[:, c, :, hb], vf.at[s, c], lsem.at[16 + 8 * s + c]))

    def rdma(src, dst, i, dev):
        return pltpu.make_async_remote_copy(src, dst, ssem.at[i], rsem.at[i], device_id=(dev,),
                                            device_id_type=pl.DeviceIdType.MESH)

    def snd_x(c):
        return rdma(xb.at[0, c], xb.at[1, c], c, pp)

    def snd_wq(g):
        return rdma(wqb.at[0, g], wqb.at[1, g], 4 + g, qq)

    def snd_wo(j):
        return rdma(wob.at[j, 0], wob.at[j, 1], 8 + j, qq)

    def snd_p(j):
        return rdma(psend.at[j], precv.at[j], 16 + j, pp)

    for t in range(4):
        ld_x(t).start()
        ld_wq(t).start()
    for c in range(4):
        for d in ld_kv(0, c):
            d.start()
    for c in range(4):
        for d in ld_kv(1, c):
            d.start()
    for g in range(4):
        ld_wo(g).start()

    def qproj(r, c, s, g):
        q = jnp.dot(xb[r, c], wqb[s, g], preferred_element_type=F32) * SCALE
        qb[r, c, s * 4 + g] = q.astype(BF)

    def attn(r, c, s, g):
        for e in range(2):
            q = qb[r, c, s * 4 + g, :, pl.ds(128 * e, 128)]
            sc = lax.dot_general(q, kb[s, c, 2 * g + e], NT, preferred_element_type=F32)
            m = jnp.max(sc, axis=1, keepdims=True)
            p = jnp.exp2(sc - m)
            l = jnp.sum(p, axis=1, keepdims=True)
            o = jnp.dot(p.astype(BF), vb[s, c, 2 * g + e], preferred_element_type=F32)
            ctx[r, s * 4 + g, c, :, pl.ds(128 * e, 128)] = (o * (1.0 / l)).astype(BF)

    def cvt_kv(s, c):
        for d in ld_kv(s, c):
            d.wait()
        for src, dst in ((kf, kb), (vf, vb)):
            flat = src.at[s, c].reshape(2048, 128)
            for h in range(8):
                dst[s, c, h] = flat[pl.ds(h, 256, stride=8), :].astype(BF)

    def oproj(r, j):
        acc = None
        for u in range(8):
            a = ctx[r, u].reshape(1024, 256)
            d = jnp.dot(a, wob[j, u // 4, pl.ds(256 * (u % 4), 256), :], preferred_element_type=F32)
            acc = d if acc is None else acc + d
        return acc

    for t in range(4):
        ld_x(t).wait()
        xb[0, t] = xf[t].reshape(256, 1024).astype(BF)
        if t == 0:
            pl.semaphore_wait(bar, 2)
        snd_x(t).start()
        ld_wq(t).wait()
        wqb[0, t] = wqf[t].astype(BF)
        snd_wq(t).start()
        for (c, g) in [(t, g) for g in range(t)] + [(c, t) for c in range(t + 1)]:
            qproj(0, c, 0, g)

    first = {}
    for i, (r, c, s, g) in enumerate(q2):
        if r == 1:
            first.setdefault(("x", c), i)
        if s == 1:
            first.setdefault(("w", g), i)
    for i, (r, c, s, g) in enumerate(a2):
        first.setdefault(("kv", s, c), i)

    def step2(i, carry):
        for key, at in first.items():
            @pl.when(i == at)
            def _():
                if key[0] == "x":
                    snd_x(key[1]).wait_recv()
                elif key[0] == "w":
                    snd_wq(key[1]).wait_recv()
                else:
                    cvt_kv(key[1], key[2])

        @pl.when(i == 24)
        def _():
            for g in range(4):
                ld_wo(g).wait()
                for e in range(2):
                    wob[2 * g + e, 0] = wof[g, :, pl.ds(128 * e, 128)].astype(BF)
                    snd_wo(2 * g + e).start()

        attn(tab[4, i], tab[5, i], tab[6, i], tab[7, i])
        qproj(tab[0, i], tab[1, i], tab[2, i], tab[3, i])
        return carry

    lax.fori_loop(0, 48, step2, 0)

    def step3(j, carry):
        snd_wo(j).wait_recv()
        psend[j] = oproj(1, j).astype(BF)
        for c in range(4):
            attn(0, c, 1, j)
        snd_p(j).start()
        return carry

    lax.fori_loop(0, 4, step3, 0)

    def st_out(j):
        return pltpu.make_async_copy(obuf.at[j].reshape(1024, 128), out_hbm.at[0, :, pl.ds(pl.multiple_of(128 * j, 128), 128)], osem.at[j])

    def partner(j):
        snd_wo(j).wait_recv()
        psend[j] = oproj(1, j).astype(BF)
        snd_p(j).start()

    def own(j):
        acc = oproj(0, j)
        snd_p(j).wait_recv()
        res = acc + precv[j].astype(F32)
        for c in range(4):
            obuf[j, :, c] = res[256 * c:256 * (c + 1)].reshape(4, 64, 128)
        st_out(j).start()

    def step4(i, carry):
        j = tab[9, i]

        @pl.when(tab[8, i] == 1)
        def _():
            partner(j)

        @pl.when(tab[8, i] == 0)
        def _():
            own(j)
        return carry

    lax.fori_loop(0, 12, step4, 0)

    for j in range(8):
        st_out(j).wait()
        snd_p(j).wait_send()
        snd_wo(j).wait_send()
    for t in range(4):
        snd_x(t).wait_send()
        snd_wq(t).wait_send()


def _table():
    kk, q2, a2, a3 = _orders()
    tab = np.zeros((10, 48), np.int32)
    tab[0:4] = np.array(q2, np.int32).T
    tab[4:8] = np.array(a2, np.int32).T
    s4 = [(1, 4), (1, 5), (0, 0), (1, 6), (0, 1), (1, 7)] + [(0, j) for j in range(2, 8)]
    tab[8:10, :12] = np.array(s4, np.int32).T
    return tab


def pallas_dist_sparse_attn_strided_qseq_b1_sq1024_skv1024_hq8_dh128_kernel(x, Wq, K_ext, V_ext, Wo):
    anyspec = pl.BlockSpec(memory_space=pl.ANY)
    out = pl.pallas_call(
        _body,
        out_shape=jax.ShapeDtypeStruct((1, 1024, 1024), F32),
        in_specs=[pl.BlockSpec(memory_space=pltpu.SMEM)] + [anyspec] * 5,
        out_specs=anyspec,
        scratch_shapes=[
            pltpu.VMEM((4, 4, 64, 1024), F32),
            pltpu.VMEM((4, 1024, 256), F32),
            pltpu.VMEM((4, 1024, 256), F32),
            pltpu.VMEM((2, 4, 4, 64, 8, 128), F32),
            pltpu.VMEM((2, 4, 4, 64, 8, 128), F32),
            pltpu.VMEM((2, 4, 256, 1024), BF),
            pltpu.VMEM((2, 4, 1024, 256), BF),
            pltpu.VMEM((8, 2, 1024, 128), BF),
            pltpu.VMEM((2, 4, 8, 256, 128), BF),
            pltpu.VMEM((2, 4, 8, 256, 128), BF),
            pltpu.VMEM((2, 4, 8, 256, 256), BF),
            pltpu.VMEM((2, 8, 4, 256, 256), BF),
            pltpu.VMEM((8, 1024, 128), BF),
            pltpu.VMEM((8, 1024, 128), BF),
            pltpu.VMEM((8, 4, 4, 64, 128), F32),
            pltpu.SemaphoreType.DMA((28,)),
            pltpu.SemaphoreType.DMA((24,)),
            pltpu.SemaphoreType.DMA((24,)),
            pltpu.SemaphoreType.DMA((8,)),
        ],
        compiler_params=pltpu.CompilerParams(collective_id=0, vmem_limit_bytes=100 * 1024 * 1024),
    )(jnp.asarray(_table()), x.reshape(4, 4, 64, 1024), Wq, K_ext.reshape(4, 4, 64, 4, 8, 128),
      V_ext.reshape(4, 4, 64, 4, 8, 128), Wo)
    return out
```

```python
import jax
import jax.numpy as jnp
from jax import lax
from jax.experimental import pallas as pl
from jax.experimental.pallas import tpu as pltpu

BF = jnp.bfloat16
F32 = jnp.float32
U32 = jnp.uint32
SCALE = 0.08838834764831843 * 1.4426950408889634
NT = (((1,), (1,)), ((), ()))
MESH = pl.DeviceIdType.MESH

X_OWN, WQ_OWN, X_REM, WQ_REM, WO_OWN, WO_REM = 0, 4, 8, 12, 16, 20
A_SLOT = (4, 5, 0, 3, 6, 7, 8)
B_SLOT = (4, 0, 8, 7, 3, 6, 5)
FIRST_Q, WIN_Q, WIN_A, MID = 15, 10, 12, 5


def _sums(q0, q1, q2, q3):
    return q0 + q3, q2 + q3, q0 + q1, q2 - q0, q1 - q3


def _words(even, odd):
    return pltpu.pack_elementwise([even, odd], packed_dtype=BF)


def _floats(words):
    return [pltpu.unpack_elementwise(words, index=n, packed_dtype=BF, unpacked_dtype=F32) for n in range(2)]


def _matrix(words):
    return pltpu.bitcast(words, BF)


def _split(v):
    return [jnp.concatenate([v[r + 8 * n:r + 8 * n + 8] for r in range(0, v.shape[0], 16)]) for n in range(2)]


def _mm(a, b):
    return jnp.dot(a, b, preferred_element_type=F32)


def _strassen(a, b):
    m0 = _mm(a(0), b(0))
    c11 = m0 + _mm(a(6), b(6))
    c22 = m0 + _mm(a(5), b(5))
    m3 = _mm(a(3), b(3))
    c11 = c11 + m3
    m1 = _mm(a(1), b(1))
    c21 = m1 + m3
    c22 = c22 - m1
    m4 = _mm(a(4), b(4))
    c11 = c11 - m4
    m2 = _mm(a(2), b(2))
    return c11, m2 + m4, c21, c22 + m2


def _orders():
    q = [(0, 0, 0, 0), (0, 0, 0, 1), (0, 1, 0, 0), (0, 1, 0, 1), (0, 2, 0, 0), (0, 2, 0, 1), (0, 0, 0, 2),
         (0, 1, 0, 2), (0, 2, 0, 2), (0, 0, 0, 3), (0, 1, 0, 3), (0, 2, 0, 3), (0, 3, 0, 0), (0, 3, 0, 1),
         (0, 3, 0, 2)]
    q += [(0, 3, 0, 3)] + [(1, 0, 0, g) for g in range(4)] + [(1, 0, 1, 0)] + [(0, c, 1, 0) for c in range(4)]
    q += [(1, 1, 0, g) for g in range(4)] + [(1, 1, 1, 0)]
    q += [(1, 0, 1, 1), (1, 1, 1, 1)] + [(0, c, 1, 1) for c in range(3)]
    q += [(1, 2, 0, g) for g in range(4)] + [(1, 2, 1, 0)]
    q += [(1, 2, 1, 1)] + [(1, c, 1, 2) for c in range(3)] + [(0, 3, 1, 1)]
    q += [(1, 3, 0, g) for g in range(4)] + [(1, 3, 1, 0)]
    q += [(1, c, 1, 3) for c in range(3)] + [(1, 3, 1, 1), (1, 3, 1, 2)]
    q += [(1, 3, 1, 3)] + [(0, c, 1, g) for c in range(4) for g in range(2, 4)]
    a = [(r, 0, 0, g) for r in range(2) for g in range(4)] + [(0, 1, 0, g) for g in range(4)]
    a += [(0, 2, 0, g) for g in range(4)] + [(1, 1, 0, 0)]
    a += [(0, 3, 0, g) for g in range(4)] + [(1, 1, 0, g) for g in range(1, 4)]
    a += [(1, 0, 1, 0), (1, 0, 1, 1), (1, 1, 1, 0), (1, 1, 1, 1)] + [(0, c, 1, g) for c in range(2) for g in range(2)]
    a += [(1, 2, 0, g) for g in range(4)]
    a += [(1, 0, 1, 2), (1, 1, 1, 2)] + [(1, 2, 1, g) for g in range(3)] + [(1, 3, 0, 0)]
    a += [(1, c, 1, 3) for c in range(3)] + [(1, 3, 0, g) for g in range(1, 4)]
    a += [(1, 3, 1, g) for g in range(4)] + [(0, c, 1, g) for c in range(2, 4) for g in range(2)]
    a += [(0, c, 1, g) for c in range(4) for g in range(2, 4)]
    assert len(set(q)) == 64 and len(set(a)) == 64 and len(q) == 64 and len(a) == 64
    for w in range(4):
        for i in range(WIN_A):
            assert a[WIN_A * w + i] in q[:FIRST_Q + WIN_Q * w + min(i, 8 + (i - 8) // 2)], (w, i)
        for i in range(WIN_Q):
            r, c, s, g = q[FIRST_Q + WIN_Q * w + i]
            assert r * c <= w and s * (g + 1) <= (w + 1 if i >= MID else w), (w, i)
    return q, a


def _pick(items, w):
    word = sum((32 * r + 8 * c + 4 * s + g) << (6 * n) for n, (r, c, s, g) in enumerate(items))
    v = lax.shift_right_logical(jnp.int32(word), 6 * w)
    return (v >> 5) & 1, (v >> 3) & 3, (v >> 2) & 1, v & 3


def _body(x_hbm, wq_hbm, k_hbm, v_hbm, wo_hbm, out_ref,
          xf, wqf, wof, kf, vf, op, qb, ca, psend, precv, lsem, ssem, rsem):
    me = lax.axis_index("i")
    pp = me ^ 1
    qq = 3 - me
    q_order, a_order = _orders()

    bar = pltpu.get_barrier_semaphore()
    for d in (pp, qq):
        pl.semaphore_signal(bar, inc=1, device_id=(d,), device_id_type=MESH)

    def ld_x(c, first=0, count=4, sem=0):
        rows = pl.ds(first, count)
        return [pltpu.make_async_copy(x_hbm.at[rows, c], xf.at[c, rows], lsem.at[sem + c])]

    def ld_w(src, dst, base, i):
        return [pltpu.make_async_copy(src.at[:, pl.ds(pl.multiple_of(256 * i + 128 * e, 128), 128)],
                                      dst.at[i, e], lsem.at[base + 2 * i + e]) for e in range(2)]

    def ld_wq(g):
        return ld_w(wq_hbm, wqf, 20, g)

    def ld_wo(j):
        return ld_w(wo_hbm, wof, 28, j)

    def ld_kv(s, c, only=None):
        heads = me + s * (qq - me)
        return [pltpu.make_async_copy(src.at[:, c, :, heads], dst.at[s, c], lsem.at[base + 8 * s + c])
                for n, (src, dst, base) in enumerate(((k_hbm, kf, 4), (v_hbm, vf, 8))) if only in (None, n)]

    def rdma(src, dst, i, dev):
        return pltpu.make_async_remote_copy(src, dst, ssem.at[i], rsem.at[i], device_id=(dev,),
                                            device_id_type=MESH)

    def snd_chunk(own, rem, i, sem, dev):
        return rdma(op.at[own + i, pl.ds(0, 4)], op.at[rem + i, pl.ds(0, 4)], sem + i, dev)

    def snd_x(c, h):
        half = pl.ds(2 * h, 2)
        return rdma(op.at[X_OWN + c, half], op.at[X_REM + c, half], 28 * h + c, pp)

    def snd_wq(g):
        return snd_chunk(WQ_OWN, WQ_REM, g, 4, qq)

    def snd_wo(j):
        return snd_chunk(WO_OWN, WO_REM, j, 8, qq)

    def snd_p(n):
        return rdma(psend.at[n], precv.at[n], 12 + n, pp)

    def put(i, rows, even, odd, slots=range(9)):
        sums = [_sums(*half) if max(slots) > 3 else () for half in (even, odd)]
        for t, pair in enumerate(zip(tuple(even) + sums[0], tuple(odd) + sums[1])):
            if t in slots:
                op[i, t, rows] = _words(*pair)

    def prep_x(c, quads=range(9)):
        for kt in range(4):
            for n in range(4):
                parts = [_split(xf[c, 2 * h + n // 2, pl.ds(32 * (n % 2), 32), pl.ds(512 * kh + 128 * kt, 128)])
                         for h in range(2 if max(quads) > 1 else 1) for kh in range(2)]
                put(X_OWN + c, pl.ds(64 * kt + 16 * n, 16), *zip(*parts), slots=quads)

    def prep_wq(g):
        for n in range(16):
            put(WQ_OWN + g, pl.ds(16 * n, 16),
                *[[wqf[g, e, pl.ds(512 * kh + 32 * n + odd, 16, stride=2), :] * SCALE
                   for kh in range(2) for e in range(2)] for odd in range(2)])

    def prep_wo(j):
        for u in range(4):
            for n in range(4):
                put(WO_OWN + j, pl.ds(64 * u + 16 * n, 16),
                    *[[wof[j, col, pl.ds(256 * u + 128 * e + 32 * n + odd, 16, stride=2), :]
                       for e in range(2) for col in range(2)] for odd in range(2)])

    def prep_remote(i):
        for n in range(16):
            rows = pl.ds(16 * n, 16)
            put(i, rows, *zip(*[_floats(op[i, t, rows]) for t in range(4)]), slots=range(4, 9))

    def slot(r, c, s, g):
        return 32 * r + 8 * c + 4 * s + g

    def qproj(item):
        r, c, s, g = item
        xi, wi = X_REM * r + c, WQ_OWN + 8 * s + g
        cs = _strassen(
            lambda t: jnp.concatenate([_matrix(op[xi, A_SLOT[t], pl.ds(64 * u, 64)]) for u in range(4)], axis=1),
            lambda t: _matrix(op[wi, B_SLOT[t]]))
        for t in range(4):
            qb[slot(*item), t % 2, pl.ds(64 * (t // 2), 64)] = _words(*_split(cs[t]))

    def head(ref, s, c, h):
        return ref.at[s, c].reshape(2048, 128)[pl.ds(h, 256, stride=8), :].astype(BF)

    def scores(item):
        r, c, s, g = item
        res = []
        for e in range(2):
            sc = lax.dot_general(_matrix(qb[slot(*item), e]), head(kf, s, c, 2 * g + e), NT, preferred_element_type=F32)
            p = jnp.exp2(sc - jnp.max(sc, axis=1, keepdims=True))
            l = jnp.sum(p, axis=1, keepdims=True)
            inv = pl.reciprocal(l, approx=True)
            res.append((p.astype(BF), inv * (2.0 - l * inv)))
        return res

    def context(item, probs):
        r, c, s, g = item
        oa, ob = [_mm(p, head(vf, s, c, 2 * g + e)) * inv for e, (p, inv) in enumerate(probs)]
        quads = (oa[:128], ob[:128], oa[128:], ob[128:])
        vals = quads + _sums(*quads)
        for t in range(7):
            ca[4 * r + c, t, 4 * s + g] = _words(*_split(vals[A_SLOT[t]]))

    def oproj(r, n):
        j, c = n // 4, n % 4
        return _strassen(
            lambda t: jnp.concatenate([_matrix(ca[4 * r + c, t, u]) for u in range(8)], axis=1),
            lambda t: jnp.concatenate([_matrix(op[i + j, B_SLOT[t]]) for i in (WO_OWN, WO_REM)], axis=0))

    def partner_unit(n):
        for t, v in enumerate(oproj(1, n)):
            psend[n, t] = _words(*_split(v))

    def own_unit(n, arrived=lambda: None):
        cs = oproj(0, n)
        arrived()
        j, c = n // 4, n % 4
        for t in range(4):
            v = _matrix(_words(*[a + b for a, b in zip(_split(cs[t]), _floats(precv[n, t]))]))
            cols = pl.ds(pl.multiple_of(256 * j + 128 * (t % 2), 128), 128)
            for h in range(2):
                rows = pl.ds(pl.multiple_of(512 * (t // 2) + 256 * h + 64 * c, 64), 64)
                out_ref[0, rows, cols] = v[64 * h:64 * h + 64]

    def start(*copies):
        for d in copies:
            d.start()

    def wait(*copies):
        for d in copies:
            d.wait()

    def wait_recv(*copies):
        for d in copies:
            d.wait_recv()

    blocks = []

    def apart(fn):
        blocks.append(fn)
        pl.when(me > -len(blocks))(fn)

    def attend(items, between):
        probs = [scores(it) for it in items]
        between()
        for it, p in zip(items, probs):
            context(it, p)

    start(*ld_x(0, 0, 2, sem=36), *ld_wq(0))

    @apart
    def _():
        wait(*ld_x(0, 0, 2, sem=36))
        start(*ld_x(0, 2, 2))
        prep_x(0, quads=(0, 1))
        pl.semaphore_wait(bar, 2)
        snd_x(0, 0).start()

    done = 0
    for n, (ld, prep, snd, upto, nxt) in enumerate([
            (ld_wq(0), lambda: prep_wq(0), [snd_wq(0)], 0, ld_wq(1)),
            (ld_x(0, 2, 2), lambda: prep_x(0, quads=range(2, 9)), [snd_x(0, 1)], 1, ld_x(1)),
            (ld_wq(1), lambda: prep_wq(1), [snd_wq(1)], 2, ld_x(2)),
            (ld_x(1), lambda: prep_x(1), [snd_x(1, 0), snd_x(1, 1)], 4, ld_wq(2)),
            (ld_x(2), lambda: prep_x(2), [snd_x(2, 0), snd_x(2, 1)], 6, ld_wq(3) + ld_x(3)),
            (ld_wq(2), lambda: prep_wq(2), [snd_wq(2)], 9, ld_kv(0, 0)),
            (ld_wq(3), lambda: prep_wq(3), [snd_wq(3)], 12, ld_kv(0, 1))]):
        @apart
        def _():
            wait(*ld)
            start(*nxt)
            prep()
            start(*snd)

        for m, item in enumerate(q_order[done:upto]):
            qproj(item)
            if n == 6 and m == 0:
                wait(*ld_x(3))
        done = upto
    prep_x(3)
    for item in q_order[done:FIRST_Q]:
        qproj(item)
    start(snd_x(3, 0), snd_x(3, 1))

    def stage2(w, carry):
        for at, old, new in [(0, ld_kv(0, 0), ld_wo(0)), (1, ld_kv(0, 2), ld_wo(1) + ld_kv(1, 0)),
                             (2, ld_kv(1, 0) + ld_kv(1, 1), ld_kv(1, 2))]:
            @pl.when(w == at)
            def _():
                wait(*old)
                start(*new)

        @apart
        def _():
            wait_recv(snd_x(w, 0), snd_x(w, 1))
            prep_remote(X_REM + w)

        qs = [_pick(q_order[FIRST_Q + i::WIN_Q][:4], w) for i in range(WIN_Q)]
        items = [_pick(a_order[i::WIN_A][:4], w) for i in range(WIN_A)]
        for i in range(WIN_Q):
            if i == MID:
                pl.when(w == 0)(lambda: start(*ld_kv(0, 2), *ld_kv(0, 3)))
                pl.when(w == 1)(lambda: start(*ld_kv(1, 1), *ld_wo(2)))
                pl.when(w == 2)(lambda: start(*ld_kv(1, 3), *ld_wo(3)))
                pl.when(w >= 2)(lambda: snd_wo(w - 2).start())

                @apart
                def _():
                    _, c, s, _ = _pick([(0, 1, 0, 0), (0, 3, 0, 0), (0, 2, 1, 0), (0, 3, 1, 0)], w)
                    wait(*ld_kv(s, c), *ld_wo(w))
                    wait_recv(snd_wq(w))
                    prep_remote(WQ_REM + w)

            first = i + max(i - 8, 0)
            attend(items[first:first + 1 + (i >= 8)], lambda: qproj(qs[i]))
        prep_wo(w)
        return carry

    lax.fori_loop(0, 4, stage2, 0)

    rest_a = a_order[4 * WIN_A:]
    rest_q = q_order[FIRST_Q + 4 * WIN_Q:]

    def slots(items, projections):
        for it, later in zip(items, projections):
            attend([it], lambda: qproj(later))

    def partner_pair(n, between=lambda f: f()):
        between(lambda: partner_unit(n))
        partner_unit(n + 1)
        start(snd_p(n), snd_p(n + 1))

    def begin_chunk(j):
        @apart
        def _():
            wait_recv(snd_wo(j))
            prep_remote(WO_REM + j)

        partner_pair(4 * j)

    attend(rest_a[0:2], lambda: qproj(rest_q[0]))
    begin_chunk(0)
    snd_wo(2).start()

    @apart
    def _():
        slots(rest_a[2:4], rest_q[1:3])
        partner_pair(2)

    apart(lambda: slots(rest_a[4:8], rest_q[3:7]))

    begin_chunk(1)
    snd_wo(3).start()

    @apart
    def _():
        attend(rest_a[8:10], lambda: qproj(rest_q[7]))
        attend(rest_a[10:11], lambda: qproj(rest_q[8]))
        partner_pair(6, lambda f: attend(rest_a[11:13], f))

    @apart
    def _():
        wait_recv(snd_p(0), snd_p(1))
        attend(rest_a[13:], lambda: own_unit(0))
        own_unit(1)

    def stage3(j, carry):
        begin_chunk(j)
        n = 6 * j - 10
        wait_recv(snd_p(n), snd_p(n + 1))
        own_unit(n)
        own_unit(n + 1)
        partner_pair(4 * j + 2)
        wait_recv(snd_p(n + 2), snd_p(n + 3), snd_p(n + 4))
        for i in range(2, 5):
            own_unit(n + i)
        own_unit(n + 5, lambda: wait_recv(snd_p(n + 5)))
        return carry

    lax.fori_loop(2, 4, stage3, 0)
    own_unit(14, lambda: wait_recv(snd_p(14)))
    own_unit(15, lambda: wait_recv(snd_p(15)))

    for n in range(16):
        snd_p(n).wait_send()
    for t in range(4):
        snd_x(t, 0).wait_send()
        snd_x(t, 1).wait_send()
        snd_wq(t).wait_send()
        snd_wo(t).wait_send()


def pallas_dist_sparse_attn_strided_qseq_b1_sq1024_skv1024_hq8_dh128_kernel(x, Wq, K_ext, V_ext, Wo):
    hbm = pl.BlockSpec(memory_space=pl.ANY)
    return pl.pallas_call(
        _body,
        out_shape=jax.ShapeDtypeStruct((1, 1024, 1024), BF),
        in_specs=[hbm] * 5,
        out_specs=pl.BlockSpec(memory_space=pltpu.VMEM),
        scratch_shapes=[
            pltpu.VMEM((4, 4, 64, 1024), F32),
            pltpu.VMEM((4, 2, 1024, 128), F32),
            pltpu.VMEM((4, 2, 1024, 128), F32),
            pltpu.VMEM((2, 4, 4, 64, 8, 128), F32),
            pltpu.VMEM((2, 4, 4, 64, 8, 128), F32),
            pltpu.VMEM((24, 9, 256, 128), U32),
            pltpu.VMEM((64, 2, 128, 128), U32),
            pltpu.VMEM((8, 7, 8, 64, 128), U32),
            pltpu.VMEM((16, 4, 64, 128), U32),
            pltpu.VMEM((16, 4, 64, 128), U32),
            pltpu.SemaphoreType.DMA((37,)),
            pltpu.SemaphoreType.DMA((32,)),
            pltpu.SemaphoreType.DMA((32,)),
        ],
        compiler_params=pltpu.CompilerParams(collective_id=0, vmem_limit_bytes=110 * 1024 * 1024),
    )(x.reshape(4, 4, 64, 1024), Wq, K_ext.reshape(4, 4, 64, 4, 8, 128),
      V_ext.reshape(4, 4, 64, 4, 8, 128), Wo)
```

```python
import jax
import jax.numpy as jnp
from jax import lax
from jax.experimental import pallas as pl
from jax.experimental.pallas import tpu as pltpu

BF = jnp.bfloat16
F32 = jnp.float32
U32 = jnp.uint32
SCALE = 0.08838834764831843 * 1.4426950408889634
NT = (((1,), (1,)), ((), ()))
MESH = pl.DeviceIdType.MESH

X_OWN, WQ_OWN, X_REM, WQ_REM, WO_OWN, WO_REM = 0, 4, 8, 12, 16, 20
A_SLOT = (4, 5, 0, 3, 6, 7, 8)
B_SLOT = (4, 0, 8, 7, 3, 6, 5)
FIRST_Q, WIN_Q, WIN_A, MID = 15, 10, 12, 5


def _sums(q0, q1, q2, q3):
    return q0 + q3, q2 + q3, q0 + q1, q2 - q0, q1 - q3


def _words(even, odd):
    return pltpu.pack_elementwise([even, odd], packed_dtype=BF)


def _floats(words):
    return [pltpu.unpack_elementwise(words, index=n, packed_dtype=BF, unpacked_dtype=F32) for n in range(2)]


def _matrix(words):
    return pltpu.bitcast(words, BF)


def _split(v):
    return [jnp.concatenate([v[r + 8 * n:r + 8 * n + 8] for r in range(0, v.shape[0], 16)]) for n in range(2)]


def _mm(a, b):
    return jnp.dot(a, b, preferred_element_type=F32)


def _strassen(a, b):
    m0 = _mm(a(0), b(0))
    c11 = m0 + _mm(a(6), b(6))
    c22 = m0 + _mm(a(5), b(5))
    m3 = _mm(a(3), b(3))
    c11 = c11 + m3
    m1 = _mm(a(1), b(1))
    c21 = m1 + m3
    c22 = c22 - m1
    m4 = _mm(a(4), b(4))
    c11 = c11 - m4
    m2 = _mm(a(2), b(2))
    return c11, m2 + m4, c21, c22 + m2


def _orders():
    q = [(0, 0, 0, 0), (0, 0, 0, 1), (0, 1, 0, 0), (0, 1, 0, 1), (0, 2, 0, 0), (0, 2, 0, 1), (0, 0, 0, 2),
         (0, 1, 0, 2), (0, 2, 0, 2), (0, 0, 0, 3), (0, 1, 0, 3), (0, 2, 0, 3), (0, 3, 0, 0), (0, 3, 0, 1),
         (0, 3, 0, 2)]
    q += [(0, 3, 0, 3)] + [(1, 0, 0, g) for g in range(4)] + [(1, 0, 1, 0)] + [(0, c, 1, 0) for c in range(4)]
    q += [(1, 1, 0, g) for g in range(4)] + [(1, 1, 1, 0)]
    q += [(1, 0, 1, 1), (1, 1, 1, 1)] + [(0, c, 1, 1) for c in range(3)]
    q += [(1, 2, 0, g) for g in range(4)] + [(1, 2, 1, 0)]
    q += [(1, 2, 1, 1)] + [(1, c, 1, 2) for c in range(3)] + [(0, 3, 1, 1)]
    q += [(1, 3, 0, g) for g in range(4)] + [(1, 3, 1, 0)]
    q += [(1, c, 1, 3) for c in range(3)] + [(1, 3, 1, 1), (1, 3, 1, 2)]
    q += [(1, 3, 1, 3)] + [(0, c, 1, g) for c in range(4) for g in range(2, 4)]
    a = [(r, 0, 0, g) for r in range(2) for g in range(4)] + [(0, 1, 0, g) for g in range(4)]
    a += [(0, 2, 0, g) for g in range(4)] + [(1, 1, 0, 0)]
    a += [(0, 3, 0, g) for g in range(4)] + [(1, 1, 0, g) for g in range(1, 4)]
    a += [(1, 0, 1, 0), (1, 0, 1, 1), (1, 1, 1, 0), (1, 1, 1, 1)] + [(0, c, 1, g) for c in range(2) for g in range(2)]
    a += [(1, 2, 0, g) for g in range(4)]
    a += [(1, 0, 1, 2), (1, 1, 1, 2)] + [(1, 2, 1, g) for g in range(3)] + [(1, 3, 0, 0)]
    a += [(1, c, 1, 3) for c in range(3)] + [(1, 3, 0, g) for g in range(1, 4)]
    a += [(1, 3, 1, g) for g in range(4)] + [(0, c, 1, g) for c in range(2, 4) for g in range(2)]
    a += [(0, c, 1, g) for c in range(4) for g in range(2, 4)]
    assert len(set(q)) == 64 and len(set(a)) == 64 and len(q) == 64 and len(a) == 64
    for w in range(4):
        for i in range(WIN_A):
            assert a[WIN_A * w + i] in q[:FIRST_Q + WIN_Q * w + min(i, 8 + (i - 8) // 2)], (w, i)
        for i in range(WIN_Q):
            r, c, s, g = q[FIRST_Q + WIN_Q * w + i]
            assert r * c <= w and s * (g + 1) <= (w + 1 if i >= MID else w), (w, i)
    return q, a


def _pick(items, w):
    word = sum((32 * r + 8 * c + 4 * s + g) << (6 * n) for n, (r, c, s, g) in enumerate(items))
    v = lax.shift_right_logical(jnp.int32(word), 6 * w)
    return (v >> 5) & 1, (v >> 3) & 3, (v >> 2) & 1, v & 3


def _body(x_hbm, wq_hbm, k_hbm, v_hbm, wo_hbm, out_ref,
          xf, wqf, wof, kf, vf, op, qb, ca, psend, precv, lsem, ssem, rsem):
    me = lax.axis_index("i")
    pp = me ^ 1
    qq = 3 - me
    q_order, a_order = _orders()

    bar = pltpu.get_barrier_semaphore()
    for d in (pp, qq):
        pl.semaphore_signal(bar, inc=1, device_id=(d,), device_id_type=MESH)

    def ld_x(c, first=0, count=4, sem=0):
        rows = pl.ds(first, count)
        return [pltpu.make_async_copy(x_hbm.at[rows, c], xf.at[c, rows], lsem.at[sem + c])]

    def ld_w(src, dst, base, i):
        return [pltpu.make_async_copy(src.at[:, pl.ds(pl.multiple_of(256 * i + 128 * e, 128), 128)],
                                      dst.at[i, e], lsem.at[base + 2 * i + e]) for e in range(2)]

    def ld_wq(g):
        return ld_w(wq_hbm, wqf, 20, g)

    def ld_wo(j):
        return ld_w(wo_hbm, wof, 28, j)

    def ld_kv(s, c, only=None):
        heads = me + s * (qq - me)
        return [pltpu.make_async_copy(src.at[:, c, :, heads], dst.at[s, c], lsem.at[base + 8 * s + c])
                for n, (src, dst, base) in enumerate(((k_hbm, kf, 4), (v_hbm, vf, 8))) if only in (None, n)]

    def rdma(src, dst, i, dev):
        return pltpu.make_async_remote_copy(src, dst, ssem.at[i], rsem.at[i], device_id=(dev,),
                                            device_id_type=MESH)

    def snd_chunk(own, rem, i, sem, dev):
        return rdma(op.at[own + i, pl.ds(0, 4)], op.at[rem + i, pl.ds(0, 4)], sem + i, dev)

    def snd_x(c, h):
        half = pl.ds(2 * h, 2)
        return rdma(op.at[X_OWN + c, half], op.at[X_REM + c, half], 28 * h + c, pp)

    def snd_wq(g):
        return snd_chunk(WQ_OWN, WQ_REM, g, 4, qq)

    def snd_wo(j):
        return snd_chunk(WO_OWN, WO_REM, j, 8, qq)

    def snd_p(n):
        return rdma(psend.at[n], precv.at[n], 12 + n, pp)

    def put(i, rows, even, odd, slots=range(9)):
        sums = [_sums(*half) if max(slots) > 3 else () for half in (even, odd)]
        for t, pair in enumerate(zip(tuple(even) + sums[0], tuple(odd) + sums[1])):
            if t in slots:
                op[i, t, rows] = _words(*pair)

    def prep_x(c, quads=range(9)):
        for kt in range(4):
            for n in range(4):
                parts = [_split(xf[c, 2 * h + n // 2, pl.ds(32 * (n % 2), 32), pl.ds(512 * kh + 128 * kt, 128)])
                         for h in range(2 if max(quads) > 1 else 1) for kh in range(2)]
                put(X_OWN + c, pl.ds(64 * kt + 16 * n, 16), *zip(*parts), slots=quads)

    def prep_wq(g):
        for n in range(16):
            put(WQ_OWN + g, pl.ds(16 * n, 16),
                *[[wqf[g, e, pl.ds(512 * kh + 32 * n + odd, 16, stride=2), :] * SCALE
                   for kh in range(2) for e in range(2)] for odd in range(2)])

    def prep_wo(j):
        for u in range(4):
            for n in range(4):
                put(WO_OWN + j, pl.ds(64 * u + 16 * n, 16),
                    *[[wof[j, col, pl.ds(256 * u + 128 * e + 32 * n + odd, 16, stride=2), :]
                       for e in range(2) for col in range(2)] for odd in range(2)])

    def prep_remote(i):
        for n in range(16):
            rows = pl.ds(16 * n, 16)
            put(i, rows, *zip(*[_floats(op[i, t, rows]) for t in range(4)]), slots=range(4, 9))

    def slot(r, c, s, g):
        return 32 * r + 8 * c + 4 * s + g

    def qproj(item):
        r, c, s, g = item
        xi, wi = X_REM * r + c, WQ_OWN + 8 * s + g
        cs = _strassen(
            lambda t: jnp.concatenate([_matrix(op[xi, A_SLOT[t], pl.ds(64 * u, 64)]) for u in range(4)], axis=1),
            lambda t: _matrix(op[wi, B_SLOT[t]]))
        for t in range(4):
            qb[slot(*item), t % 2, pl.ds(64 * (t // 2), 64)] = _words(*_split(cs[t]))

    def head(ref, s, c, h):
        return ref.at[s, c].reshape(2048, 128)[pl.ds(h, 256, stride=8), :].astype(BF)

    def scores(item):
        r, c, s, g = item
        res = []
        for e in range(2):
            sc = lax.dot_general(_matrix(qb[slot(*item), e]), head(kf, s, c, 2 * g + e), NT, preferred_element_type=F32)
            p = jnp.exp2(sc - jnp.max(sc, axis=1, keepdims=True))
            l = jnp.sum(p, axis=1, keepdims=True)
            inv = pl.reciprocal(l, approx=True)
            res.append((p.astype(BF), inv * (2.0 - l * inv)))
        return res

    def context(item, probs):
        r, c, s, g = item
        oa, ob = [_mm(p, head(vf, s, c, 2 * g + e)) * inv for e, (p, inv) in enumerate(probs)]
        quads = (oa[:128], ob[:128], oa[128:], ob[128:])
        vals = quads + _sums(*quads)
        for t in range(7):
            ca[4 * r + c, t, 4 * s + g] = _words(*_split(vals[A_SLOT[t]]))

    def oproj(r, n):
        j, c = n // 4, n % 4
        return _strassen(
            lambda t: jnp.concatenate([_matrix(ca[4 * r + c, t, u]) for u in range(8)], axis=1),
            lambda t: jnp.concatenate([_matrix(op[i + j, B_SLOT[t]]) for i in (WO_OWN, WO_REM)], axis=0))

    def partner_unit(n):
        for t, v in enumerate(oproj(1, n)):
            psend[n, t] = _words(*_split(v))

    def own_unit(n):
        cs = oproj(0, n)
        j, c = n // 4, n % 4
        for t in range(4):
            v = _matrix(_words(*[a + b for a, b in zip(_split(cs[t]), _floats(precv[n, t]))]))
            cols = pl.ds(pl.multiple_of(256 * j + 128 * (t % 2), 128), 128)
            for h in range(2):
                rows = pl.ds(pl.multiple_of(512 * (t // 2) + 256 * h + 64 * c, 64), 64)
                out_ref[0, rows, cols] = v[64 * h:64 * h + 64]

    def start(*copies):
        for d in copies:
            d.start()

    def wait(*copies):
        for d in copies:
            d.wait()

    def wait_recv(*copies):
        for d in copies:
            d.wait_recv()

    blocks = []

    def apart(fn):
        blocks.append(fn)
        pl.when(me > -len(blocks))(fn)

    def attend(items, between):
        probs = [scores(it) for it in items]
        between()
        for it, p in zip(items, probs):
            context(it, p)

    start(*ld_x(0, 0, 2, sem=36), *ld_wq(0))

    @apart
    def _():
        wait(*ld_x(0, 0, 2, sem=36))
        start(*ld_x(0, 2, 2))
        prep_x(0, quads=(0, 1))
        pl.semaphore_wait(bar, 2)
        snd_x(0, 0).start()

    done = 0
    for n, (ld, prep, snd, upto, nxt) in enumerate([
            (ld_wq(0), lambda: prep_wq(0), [snd_wq(0)], 0, ld_wq(1)),
            (ld_x(0, 2, 2), lambda: prep_x(0, quads=range(2, 9)), [snd_x(0, 1)], 1, ld_x(1)),
            (ld_wq(1), lambda: prep_wq(1), [snd_wq(1)], 2, ld_x(2)),
            (ld_x(1), lambda: prep_x(1), [snd_x(1, 0), snd_x(1, 1)], 4, ld_wq(2)),
            (ld_x(2), lambda: prep_x(2), [snd_x(2, 0), snd_x(2, 1)], 6, ld_wq(3) + ld_x(3)),
            (ld_wq(2), lambda: prep_wq(2), [snd_wq(2)], 9, ld_kv(0, 0)),
            (ld_wq(3), lambda: prep_wq(3), [snd_wq(3)], 12, ld_kv(0, 1))]):
        @apart
        def _():
            wait(*ld)
            start(*nxt)
            prep()
            start(*snd)

        for m, item in enumerate(q_order[done:upto]):
            qproj(item)
            if n == 6 and m == 0:
                wait(*ld_x(3))
        done = upto
    prep_x(3)
    for item in q_order[done:FIRST_Q]:
        qproj(item)
    start(snd_x(3, 0), snd_x(3, 1))

    def stage2(w, carry):
        for at, old, new in [(0, ld_kv(0, 0), ld_wo(0)), (1, ld_kv(0, 2), ld_wo(1) + ld_kv(1, 0, 0)),
                             (2, ld_kv(1, 0) + ld_kv(1, 1), ld_kv(1, 2))]:
            @pl.when(w == at)
            def _():
                wait(*old)
                start(*new)

        @apart
        def _():
            wait_recv(snd_x(w, 0), snd_x(w, 1))
            prep_remote(X_REM + w)

        for i in range(WIN_Q):
            if i == MID:
                pl.when(w == 0)(lambda: start(*ld_kv(0, 2), *ld_kv(0, 3)))
                pl.when(w == 1)(lambda: start(*ld_kv(1, 0, 1), *ld_kv(1, 1), *ld_wo(2)))
                pl.when(w == 2)(lambda: start(*ld_kv(1, 3), *ld_wo(3)))
                pl.when(w >= 2)(lambda: snd_wo(w - 2).start())

                @apart
                def _():
                    _, c, s, _ = _pick([(0, 1, 0, 0), (0, 3, 0, 0), (0, 2, 1, 0), (0, 3, 1, 0)], w)
                    wait(*ld_kv(s, c), *ld_wo(w))
                    wait_recv(snd_wq(w))
                    prep_remote(WQ_REM + w)

            if i == 7:
                prep_wo(w)
            first = i + max(i - 8, 0)
            attend([_pick(a_order[first + m::WIN_A][:4], w) for m in range(1 + (i >= 8))],
                   lambda: qproj(_pick(q_order[FIRST_Q + i::WIN_Q][:4], w)))
        return carry

    lax.fori_loop(0, 4, stage2, 0)

    rest_a = a_order[4 * WIN_A:]
    rest_q = q_order[FIRST_Q + 4 * WIN_Q:]

    def slots(items, projections):
        for it, later in zip(items, projections):
            attend([it], lambda: qproj(later))

    def partner_pair(n, between=lambda f: f()):
        between(lambda: partner_unit(n))
        partner_unit(n + 1)
        start(snd_p(n), snd_p(n + 1))

    def own_units(n, count):
        wait_recv(*[snd_p(n + i) for i in range(count)])
        for i in range(count):
            own_unit(n + i)

    def begin_chunk(j):
        @apart
        def _():
            wait_recv(snd_wo(j))
            prep_remote(WO_REM + j)

        if isinstance(j, int):
            partner_pair(4 * j)
        else:
            for n in (4 * j, 4 * j + 1):
                partner_unit(n)
                snd_p(n).start()

    attend(rest_a[0:2], lambda: qproj(rest_q[0]))
    begin_chunk(0)
    snd_wo(2).start()

    @apart
    def _():
        slots(rest_a[2:4], rest_q[1:3])
        partner_pair(2)

    apart(lambda: slots(rest_a[4:8], rest_q[3:7]))

    begin_chunk(1)
    snd_wo(3).start()

    @apart
    def _():
        attend(rest_a[8:10], lambda: qproj(rest_q[7]))
        attend(rest_a[10:11], lambda: qproj(rest_q[8]))
        partner_pair(6, lambda f: attend(rest_a[11:13], f))

    @apart
    def _():
        wait_recv(snd_p(0))
        attend(rest_a[13:], lambda: own_unit(0))

    def stage3(j, carry):
        begin_chunk(j)
        own_units(6 * j - 11, 2)
        partner_pair(4 * j + 2)
        own_units(6 * j - 9, 4)
        return carry

    lax.fori_loop(2, 4, stage3, 0)
    own_units(13, 2)
    own_units(15, 1)

    for n in range(16):
        snd_p(n).wait_send()
    for t in range(4):
        snd_x(t, 0).wait_send()
        snd_x(t, 1).wait_send()
        snd_wq(t).wait_send()
        snd_wo(t).wait_send()


def pallas_dist_sparse_attn_strided_qseq_b1_sq1024_skv1024_hq8_dh128_kernel(x, Wq, K_ext, V_ext, Wo):
    hbm = pl.BlockSpec(memory_space=pl.ANY)
    return pl.pallas_call(
        _body,
        out_shape=jax.ShapeDtypeStruct((1, 1024, 1024), BF),
        in_specs=[hbm] * 5,
        out_specs=pl.BlockSpec(memory_space=pltpu.VMEM),
        scratch_shapes=[
            pltpu.VMEM((4, 4, 64, 1024), F32),
            pltpu.VMEM((4, 2, 1024, 128), F32),
            pltpu.VMEM((4, 2, 1024, 128), F32),
            pltpu.VMEM((2, 4, 4, 64, 8, 128), F32),
            pltpu.VMEM((2, 4, 4, 64, 8, 128), F32),
            pltpu.VMEM((24, 9, 256, 128), U32),
            pltpu.VMEM((64, 2, 128, 128), U32),
            pltpu.VMEM((8, 7, 8, 64, 128), U32),
            pltpu.VMEM((16, 4, 64, 128), U32),
            pltpu.VMEM((16, 4, 64, 128), U32),
            pltpu.SemaphoreType.DMA((37,)),
            pltpu.SemaphoreType.DMA((32,)),
            pltpu.SemaphoreType.DMA((32,)),
        ],
        compiler_params=pltpu.CompilerParams(collective_id=0, vmem_limit_bytes=110 * 1024 * 1024),
    )(x.reshape(4, 4, 64, 1024), Wq, K_ext.reshape(4, 4, 64, 4, 8, 128),
      V_ext.reshape(4, 4, 64, 4, 8, 128), Wo)
```
